```python
import numpy as np

kernel_name = "dist_layernorm_xy_m512_n256"

def setup_inputs():
    x = np.random.randn(1024, 512).astype(np.float32)
    gamma = np.random.randn(512).astype(np.float32)
    beta = np.random.randn(512).astype(np.float32)
    return {"x": x, "gamma": gamma, "beta": beta}

def reference(x: np.ndarray, gamma: np.ndarray, beta: np.ndarray) -> np.ndarray:
    eps = 1e-5
    mean = np.mean(x, axis=1, keepdims=True)
    var = np.var(x, axis=1, keepdims=True)
    return gamma * (x - mean) / np.sqrt(var + eps) + beta
```

```python
import jax
import jax.numpy as jnp
from jax import lax
from jax.experimental import pallas as pl
from jax.experimental.pallas import tpu as pltpu

EPS = 1e-5


def pallas_dist_layernorm_xy_m512_n256_kernel(
    x: jax.Array,
    gamma: jax.Array,
    beta: jax.Array,
):
    m, n = x.shape

    def kernel_body(x_ref, g_ref, b_ref, o_ref, send_buf, recv_buf, send_sem, recv_sem):
        my_x = lax.axis_index("x")
        my_y = lax.axis_index("y")
        peer = (my_x, 1 - my_y)

        barrier = pltpu.get_barrier_semaphore()
        pl.semaphore_signal(
            barrier, inc=1, device_id=peer, device_id_type=pl.DeviceIdType.MESH
        )

        xv = x_ref[...]
        mean = jnp.sum(xv, axis=1, keepdims=True) * (1.0 / n)
        d = xv - mean
        m2 = jnp.sum(d * d, axis=1, keepdims=True)
        lane = lax.broadcasted_iota(jnp.int32, (m, 128), 1)
        packed = jnp.where(lane == 0, mean, jnp.where(lane == 1, m2, 0.0))
        send_buf[...] = packed.T[0:8, :]

        pl.semaphore_wait(barrier, 1)
        rdma = pltpu.make_async_remote_copy(
            src_ref=send_buf,
            dst_ref=recv_buf,
            send_sem=send_sem,
            recv_sem=recv_sem,
            device_id=peer,
            device_id_type=pl.DeviceIdType.MESH,
        )
        rdma.start()
        rdma.wait()

        other = jnp.concatenate(
            [recv_buf[...], jnp.zeros((120, m), jnp.float32)], axis=0
        ).T
        mean_o = other[:, 0:1]
        m2_o = other[:, 1:2]
        delta = mean - mean_o
        var = (m2 + m2_o + delta * delta * (n / 2)) * (1.0 / (2 * n))
        rstd = lax.rsqrt(var + EPS)
        o_ref[...] = (d + 0.5 * delta) * rstd * g_ref[...] + b_ref[...]

    vmem = pl.BlockSpec(memory_space=pltpu.VMEM)
    return pl.pallas_call(
        kernel_body,
        out_shape=jax.ShapeDtypeStruct((m, n), jnp.float32),
        in_specs=[vmem, vmem, vmem],
        out_specs=vmem,
        scratch_shapes=[
            pltpu.VMEM((8, m), jnp.float32),
            pltpu.VMEM((8, m), jnp.float32),
            pltpu.SemaphoreType.DMA,
            pltpu.SemaphoreType.DMA,
        ],
        compiler_params=pltpu.CompilerParams(collective_id=0),
    )(x, gamma.reshape(1, n), beta.reshape(1, n))
```

```python
import jax
import jax.numpy as jnp
from jax import lax
from jax.experimental import pallas as pl
from jax.experimental.pallas import tpu as pltpu

EPS = 1e-5
TILE = (8, 128)
GROUPS = 16
BLOCKS = 4
LAST = BLOCKS - 1

LOADS = (
    (0, 48, 64), (0, 16, 32), (0, 0, 16),
    (1, 0, 16), (1, 16, 24), (1, 24, 28), (1, 28, 32),
    (0, 32, 40), (0, 40, 44), (0, 44, 48),
    (1, 32, 40), (1, 40, 44), (1, 44, 48),
    (1, 48, 50), (1, 50, 52), (1, 52, 54), (1, 54, 56), (1, 56, 58),
    (1, 58, 60), (1, 60, 62), (1, 62, 63), (1, 63, 64),
)


def _bits(v):
    return pltpu.bitcast(v, jnp.int32)


def _floats(v):
    return pltpu.bitcast(v, jnp.float32)


def _pack(lo, hi):
    lo = lax.shift_right_logical(_bits(lo) + 0x8000, 16)
    return ((_bits(hi) + 0x8000 - lo) & -0x10000) | lo


def _unpack(word):
    return _floats(word << 16), _floats(word)


def _inverse_root(v):
    return jnp.exp2(jnp.log2(v) * -0.5)


def _row_sum(v):
    return jnp.broadcast_to(jnp.sum(v, axis=1, keepdims=True), TILE)


def _rows(group):
    return pl.ds(8 * group, 8)


def _groups(block):
    return range(GROUPS * block, GROUPS * (block + 1))


def _lane(group):
    return 120 - 8 * (group % GROUPS)


def _layernorm_body(
    x_hbm, gamma_hbm, beta_hbm, out_ref,
    x_ref, gamma_ref, beta_ref, shift_ref, scaled_ref,
    partial_ref, lane_mask, outbox, inbox, scalar_inbox,
    load_sems, param_sems, fence_sem, send_sems, recv_sems,
):
    halves = (pl.ds(0, 128), pl.ds(128, 128))
    left, right = halves

    loads = []
    for i, (half, first, end) in enumerate(LOADS):
        window = (pl.ds(8 * first, 8 * (end - first)), halves[half])
        loads.append(
            pltpu.make_async_copy(x_hbm.at[window], x_ref.at[window], load_sems.at[i])
        )
        loads[i].start()
    params = (
        pltpu.make_async_copy(gamma_hbm, gamma_ref, param_sems.at[0]),
        pltpu.make_async_copy(beta_hbm, beta_ref, param_sems.at[1]),
    )

    peer = dict(
        device_id=(lax.axis_index("x"), 1 - lax.axis_index("y")),
        device_id_type=pl.DeviceIdType.MESH,
    )
    barrier = pltpu.get_barrier_semaphore()
    pl.semaphore_signal(barrier, inc=1, **peer)

    messages = [
        pltpu.make_async_remote_copy(
            outbox.at[pl.ds(i, 1)],
            scalar_inbox if i == BLOCKS + LAST else inbox.at[pl.ds(i, 1)],
            send_sems.at[i],
            recv_sems.at[i],
            **peer,
        )
        for i in range(2 * BLOCKS)
    ]

    sublane = lax.broadcasted_iota(jnp.int32, TILE, 0)
    diagonal = lax.broadcasted_iota(jnp.int32, TILE, 1) - sublane
    shifts, terms = {}, {}

    def fence():
        pl.semaphore_signal(fence_sem, 1)
        pl.semaphore_wait(fence_sem, 1)

    def consume(i):
        half, first, end = LOADS[i]
        for g in range(first, end):
            if half == 0:
                shifts[g] = _row_sum(x_ref[_rows(g), left] * (1.0 / 128))
            else:
                k = shift_ref[_rows(g), :]
                a, b = x_ref[_rows(g), left] - k, x_ref[_rows(g), right] - k
                terms[g] = b + a, b * b + (a * a + 2 * EPS)

    def await_loads(first, end):
        for i in range(first, end):
            loads[i].wait()
            consume(i)

    def keep_shifts(block):
        for g in _groups(block):
            shift_ref[_rows(g), :] = shifts[g]

    def send(i, row):
        outbox[pl.ds(i, 1), :] = row
        messages[i].start()

    def send_shifts(block):
        placed = jnp.zeros(TILE, jnp.float32)
        for g in _groups(block):
            placed = jnp.where(diagonal == _lane(g), shifts[g], placed)
        send(block, _bits(jnp.sum(placed, axis=0, keepdims=True)))

    def moments(block):
        w, s = (
            lax.dot_general(
                jnp.full(TILE, weight, jnp.float32),
                jnp.concatenate([terms[g][j] for g in reversed(_groups(block))]),
                (((1,), (1,)), ((), ())),
                preferred_element_type=jnp.float32,
            )
            for j, weight in enumerate((1.0 / 32, 1.0 / 2))
        )
        return _pack(w, s)[0:1]

    loads[0].wait()
    for copy in params:
        copy.start()
    pl.semaphore_wait(barrier, 1)
    consume(0)
    await_loads(1, 2)
    keep_shifts(3)
    await_loads(2, 3)
    send_shifts(3)
    keep_shifts(0)
    await_loads(3, 4)
    moments0 = moments(0)
    keep_shifts(1)
    send_shifts(0)
    send_shifts(1)
    await_loads(4, 7)
    moments1 = moments(1)
    send(BLOCKS + 0, moments0)
    await_loads(7, 10)
    send(BLOCKS + 1, moments1)
    keep_shifts(2)
    await_loads(10, 13)
    send_shifts(2)
    moments2 = moments(2)
    await_loads(13, len(LOADS))
    moments3 = moments(3)
    send(BLOCKS + 2, moments2)
    send(BLOCKS + 3, moments3)

    fence()
    for copy in params:
        copy.wait()
    gammas = [jnp.broadcast_to(gamma_ref[:, h], TILE) for h in halves]
    betas = [jnp.broadcast_to(beta_ref[:, h], TILE) for h in halves]
    for g in range(BLOCKS * GROUPS):
        k = shift_ref[_rows(g), :]
        for h, gamma in zip(halves, gammas):
            scaled_ref[_rows(g), h] = (x_ref[_rows(g), h] - k) * (gamma * 16.0)
    for g in range(GROUPS):
        lane_mask[g] = jnp.where(diagonal == _lane(g), -1, 0)
    for message in messages:
        message.wait_send()
    fence()

    def message_row(box, i):
        return jnp.broadcast_to(box[pl.ds(i, 1), :], TILE)

    def shift_gap(block):
        return 8.0 * (
            _floats(message_row(inbox, block)) - _floats(message_row(outbox, block))
        )

    def spread(lanes, group):
        return _bits(_row_sum(_floats(lanes & lane_mask[group % GROUPS])))

    def receive(block):
        messages[block].wait_recv()
        messages[BLOCKS + block].wait_recv()

    def combine(block):
        gap = shift_gap(block)
        w, s = _unpack(message_row(outbox, BLOCKS + block))
        wp, sp = _unpack(message_row(inbox, BLOCKS + block))
        c = gap + (wp - w)
        v = ((s + sp) - 2.0 * (w * w + wp * wp)) + c * c
        return _pack(gap + (wp + w), _inverse_root(v))

    def normalize(group, u, r):
        parts = [
            (scaled_ref[_rows(group), h] - u * gamma) * r + beta
            for h, gamma, beta in zip(halves, gammas, betas)
        ]
        out_ref[_rows(group), :] = jnp.concatenate(parts, axis=1).astype(out_ref.dtype)

    def finish(block, combined):
        for g in _groups(block):
            normalize(g, *_unpack(spread(combined, g)))

    messages[LAST].wait_recv()
    gap = shift_gap(LAST)
    w, s = _unpack(message_row(outbox, BLOCKS + LAST))
    c = gap - w
    partial = _pack(2.0 * c, s - 2.0 * w * w + c * c)
    for i, g in enumerate(_groups(LAST)):
        partial_ref[0, i], partial_ref[1, i] = _unpack(spread(partial, g))
        u = _floats(spread(_bits(gap + w), g))
        for h, gamma in zip(halves, gammas):
            scaled_ref[_rows(g), h] -= u * gamma
    fence()
    receive(0)
    combined0 = combine(0)
    fence()
    receive(1)
    combined1 = combine(1)
    finish(0, combined0)
    finish(1, combined1)
    fence()
    receive(2)
    messages[BLOCKS + LAST].wait_recv()
    finish(2, combine(2))
    words = sublane
    for i, g in enumerate(_groups(LAST)):
        for j in range(8):
            words = jnp.where(sublane == j, scalar_inbox[0, _lane(g) + j], words)
        wp, sp = _unpack(words)
        slope, base = partial_ref[0, i], partial_ref[1, i]
        normalize(g, wp, _inverse_root((base + sp) + wp * (slope - wp)))


def pallas_dist_layernorm_xy_m512_n256_kernel(
    x: jax.Array,
    gamma: jax.Array,
    beta: jax.Array,
):
    m, n = x.shape
    assert (m, n) == (8 * GROUPS * BLOCKS, 256)
    hbm = pl.BlockSpec(memory_space=pltpu.HBM)
    return pl.pallas_call(
        _layernorm_body,
        out_shape=jax.ShapeDtypeStruct((m, n), jnp.bfloat16),
        in_specs=[hbm, hbm, hbm],
        out_specs=pl.BlockSpec(memory_space=pltpu.VMEM),
        scratch_shapes=[
            pltpu.VMEM((m, n), jnp.float32),
            pltpu.VMEM((1, n), jnp.float32),
            pltpu.VMEM((1, n), jnp.float32),
            pltpu.VMEM((m, 128), jnp.float32),
            pltpu.VMEM((m, n), jnp.float32),
            pltpu.VMEM((2, GROUPS, *TILE), jnp.float32),
            pltpu.VMEM((GROUPS, *TILE), jnp.int32),
            pltpu.VMEM((2 * BLOCKS, 128), jnp.int32),
            pltpu.VMEM((2 * BLOCKS, 128), jnp.int32),
            pltpu.SMEM((1, 128), jnp.int32),
            pltpu.SemaphoreType.DMA((len(LOADS),)),
            pltpu.SemaphoreType.DMA((2,)),
            pltpu.SemaphoreType.REGULAR,
            pltpu.SemaphoreType.DMA((2 * BLOCKS,)),
            pltpu.SemaphoreType.DMA((2 * BLOCKS,)),
        ],
        compiler_params=pltpu.CompilerParams(
            collective_id=0,
            disable_bounds_checks=True,
            disable_semaphore_checks=True,
            flags={
                "XLA_TPU_RESCHEDULE_DMA_DONES": True,
                "XLA_TPU_FORCE_LP_LLO_SCHEDULER": True,
            },
        ),
    )(x, gamma.reshape(1, n), beta.reshape(1, n))
```
